```python
import numpy as np

kernel_name = "dist_sum_ax1_xy_m512_n256"

def setup_inputs():
    return {"x": np.random.randn(1024, 512).astype(np.float32)}

def reference(x: np.ndarray) -> np.ndarray:
    return np.sum(x, axis=1, keepdims=True)
```

```python
import jax
import jax.numpy as jnp
from jax import lax
from jax.experimental import pallas as pl
from jax.experimental.pallas import tpu as pltpu


def pallas_dist_sum_ax1_xy_m512_n256_kernel(x: jax.Array):
    m, n = x.shape

    def body(x_ref, out_ref, send_buf, recv_buf, send_sem, recv_sem):
        my_x = lax.axis_index("x")
        my_y = lax.axis_index("y")
        peer = (my_x, 1 - my_y)

        barrier = pltpu.get_barrier_semaphore()
        pl.semaphore_signal(barrier, inc=1, device_id=peer,
                            device_id_type=pl.DeviceIdType.MESH)

        xs = x_ref[...]
        part = jnp.sum((xs[:, :128] + xs[:, 128:]).T, axis=0, keepdims=True)
        send_buf[...] = part

        pl.semaphore_wait(barrier, 1)
        rdma = pltpu.make_async_remote_copy(
            src_ref=send_buf, dst_ref=recv_buf, send_sem=send_sem,
            recv_sem=recv_sem, device_id=peer,
            device_id_type=pl.DeviceIdType.MESH)
        rdma.start()
        rdma.wait_recv()
        out_ref[...] = part + recv_buf[...]
        rdma.wait_send()

    out = pl.pallas_call(
        body,
        out_shape=jax.ShapeDtypeStruct((1, m), x.dtype),
        in_specs=[pl.BlockSpec(memory_space=pltpu.VMEM)],
        out_specs=pl.BlockSpec(memory_space=pltpu.VMEM),
        scratch_shapes=[
            pltpu.VMEM((1, m), jnp.float32),
            pltpu.VMEM((1, m), jnp.float32),
            pltpu.SemaphoreType.DMA,
            pltpu.SemaphoreType.DMA,
        ],
        compiler_params=pltpu.CompilerParams(collective_id=0),
    )(x)
    return out.reshape(m, 1)
```

```python
import jax
import jax.numpy as jnp
from jax import lax
from jax.experimental import pallas as pl
from jax.experimental.pallas import tpu as pltpu

SUBLANES, LANES = 8, 128
RAW_ROWS = 40
CHUNK_ENDS = (208, 304, 384)


def _merge(slabs, lane_slab):
    if len(slabs) == 1:
        return slabs[0][1]
    half = len(slabs) // 2
    return jnp.where(
        lane_slab >= slabs[half][0],
        _merge(slabs[half:], lane_slab),
        _merge(slabs[:half], lane_slab),
    )


def pallas_dist_sum_ax1_xy_m512_n256_kernel(x: jax.Array):
    m, n = x.shape
    split = m - RAW_ROWS
    edges = (0, *CHUNK_ENDS, split)
    n_chunks = len(edges) - 1
    last = m // LANES - 1

    def body(x_hbm, out_ref, x_buf, raw_buf, send_buf, recv_buf,
             load_sems, send_sems, recv_sems):
        def load(lo, hi, i):
            rows = pl.ds(lo, hi - lo)
            return pltpu.make_async_copy(x_hbm.at[rows], x_buf.at[rows], load_sems.at[i])

        loads = [load(edges[i], edges[i + 1], i) for i in range(n_chunks)]
        for copy in loads:
            copy.start(priority=1)

        peer = (lax.axis_index("x"), 1 - lax.axis_index("y"))

        def to_peer(src, dst, i):
            return pltpu.make_async_remote_copy(
                src, dst, send_sems.at[i], recv_sems.at[i],
                device_id=peer, device_id_type=pl.DeviceIdType.MESH)

        head, tail = pl.ds(0, last * LANES), pl.ds(last * LANES, LANES)
        raw_msg = to_peer(x_hbm.at[pl.ds(split, RAW_ROWS)], raw_buf, 0)
        head_msg = to_peer(send_buf.at[:, head], recv_buf.at[:, head], 1)
        tail_msg = to_peer(send_buf.at[:, tail], recv_buf.at[:, tail], 2)

        barrier = pltpu.get_barrier_semaphore()
        pl.semaphore_signal(barrier, inc=1, device_id=peer,
                            device_id_type=pl.DeviceIdType.MESH)
        pl.semaphore_wait(barrier, 1)
        raw_msg.start()

        lane = lax.broadcasted_iota(jnp.int32, (SUBLANES, LANES), 1)
        lane_slab, lane_row = lane >> 3, lane & 7

        def fold(ref, r):
            return sum(ref[r:r + SUBLANES, c:c + LANES] for c in range(0, n, LANES))

        def slab(r, folded):
            total = jnp.sum(folded, axis=1, keepdims=True)
            return (r % LANES) // SUBLANES, jnp.broadcast_to(total, (SUBLANES, LANES))

        def to_lanes(merged):
            return jnp.take_along_axis(merged, lane_row, axis=0)[:1]

        mine, merged = [], None
        for i, copy in enumerate(loads):
            copy.wait()
            slabs = []
            for r in range(edges[i], edges[i + 1], SUBLANES):
                slabs.append(slab(r, fold(x_buf, r)))
                end = r + SUBLANES
                if end % LANES == 0 or end == edges[i + 1]:
                    new, first = _merge(slabs, lane_slab), slabs[0][0]
                    merged = jnp.where(lane_slab >= first, new, merged) if first else new
                    slabs = []
                if end % LANES == 0 or end == split:
                    g = r // LANES
                    mine.append(to_lanes(merged))
                    send_buf[:, g * LANES:(g + 1) * LANES] = mine[g]
            if edges[i + 1] == last * LANES:
                head_msg.start()
        tail_msg.start()

        raw_load = load(split, m, n_chunks)
        raw_load.start()
        raw_load.wait()
        for msg in (head_msg, tail_msg, raw_msg):
            msg.wait_send()

        raw_rows = range(split, m, SUBLANES)
        own = [fold(x_buf, r) for r in raw_rows]
        raw_msg.wait_recv()
        both = to_lanes(_merge(
            [slab(r, v + fold(raw_buf, r - split)) for r, v in zip(raw_rows, own)],
            lane_slab))

        head_msg.wait_recv()
        for g in range(last):
            cols = slice(g * LANES, (g + 1) * LANES)
            out_ref[:, cols] = mine[g] + recv_buf[:, cols]

        tail_msg.wait_recv()
        cols = slice(last * LANES, m)
        out_ref[:, cols] = jnp.where(
            lane[:1] >= split % LANES, both, mine[last] + recv_buf[:, cols])

    out = pl.pallas_call(
        body,
        out_shape=jax.ShapeDtypeStruct((1, m), x.dtype),
        in_specs=[pl.BlockSpec(memory_space=pltpu.HBM)],
        out_specs=pl.BlockSpec(memory_space=pltpu.VMEM),
        scratch_shapes=[
            pltpu.VMEM((m, n), x.dtype),
            pltpu.VMEM((RAW_ROWS, n), x.dtype),
            pltpu.VMEM((1, m), x.dtype),
            pltpu.VMEM((1, m), x.dtype),
            pltpu.SemaphoreType.DMA((n_chunks + 1,)),
            pltpu.SemaphoreType.DMA((3,)),
            pltpu.SemaphoreType.DMA((3,)),
        ],
        compiler_params=pltpu.CompilerParams(
            collective_id=0,
            disable_bounds_checks=True,
            disable_semaphore_checks=True,
        ),
    )(x)
    return out.reshape(m, 1)
```

```python
import functools

import jax
import jax.numpy as jnp
from jax import lax
from jax.experimental import pallas as pl
from jax.experimental.pallas import tpu as pltpu

SUBLANES, LANES = 8, 128

OVERLAP_WAITS = jax.__version_info__ >= (0, 12)

RAW_ENDS = (24, 32)
CHUNK_ENDS = (
    (272, 384, 432, 456, 480, 496, 504, 512) if OVERLAP_WAITS else (272, 352, 440, 512)
)


def _merge(slabs, lane_slab):
    if len(slabs) == 1:
        return slabs[0][1]
    half = len(slabs) // 2
    return jnp.where(
        lane_slab >= slabs[half][0],
        _merge(slabs[half:], lane_slab),
        _merge(slabs[:half], lane_slab),
    )


def _kernel(x_hbm, out_ref, x_buf, raw_buf, send_buf, recv_buf,
            load_sems, send_sems, recv_sems, fence_sem):
    m, n = x_hbm.shape
    n_raw = RAW_ENDS[-1]
    chunks = list(zip((n_raw, *CHUNK_ENDS), CHUNK_ENDS))
    raw_pieces = list(zip((0, *RAW_ENDS), RAW_ENDS))
    tail = m - LANES

    def load(lo, hi, i):
        rows = pl.ds(lo, hi - lo)
        return pltpu.make_async_copy(x_hbm.at[rows], x_buf.at[rows], load_sems.at[i])

    loads = [load(lo, hi, i) for i, (lo, hi) in enumerate(chunks)]
    for copy in loads:
        copy.start()

    peer = (lax.axis_index("x"), 1 - lax.axis_index("y"))

    def to_peer(src, dst, i):
        return pltpu.make_async_remote_copy(
            src, dst, send_sems.at[i], recv_sems.at[i],
            device_id=peer, device_id_type=pl.DeviceIdType.MESH)

    head_msg, tail_msg = [
        to_peer(send_buf.at[:, cols], recv_buf.at[:, cols], i)
        for i, cols in enumerate((pl.ds(0, tail), pl.ds(tail, LANES)))
    ]
    raw_msgs = [
        to_peer(x_hbm.at[pl.ds(lo, hi - lo)], raw_buf.at[pl.ds(lo, hi - lo)], 2 + i)
        for i, (lo, hi) in enumerate(raw_pieces)
    ]

    barrier = pltpu.get_barrier_semaphore()
    pl.semaphore_signal(barrier, device_id=peer, device_id_type=pl.DeviceIdType.MESH)
    pl.semaphore_wait(barrier)
    raw_msgs[0].start()

    lane = lax.broadcasted_iota(jnp.int32, (SUBLANES, LANES), 1)
    lane_slab, lane_row = lane >> 3, lane & 7

    def fold(ref, r):
        tiles = [ref[r:r + SUBLANES, c:c + LANES] for c in range(0, n, LANES)]
        return functools.reduce(jnp.add, tiles)

    def slab(r, folded):
        sums = jnp.sum(folded, axis=1, keepdims=True)
        return r % LANES // SUBLANES, jnp.broadcast_to(sums, (SUBLANES, LANES))

    def to_lanes(merged):
        return jnp.take_along_axis(merged, lane_row, axis=0)[:1]

    def fence():
        pl.semaphore_signal(fence_sem)

    mine, merged, n_fences = [], None, 0
    for copy, (lo, hi) in zip(loads, chunks):
        copy.wait()
        if lo == n_raw:
            raw_msgs[1].start()
        slabs = []
        for r in range(lo, hi, SUBLANES):
            folded = fold(x_buf, r)
            if lo >= tail and hi < m:
                x_buf[r:r + SUBLANES, :LANES] = folded
            slabs.append(slab(r, folded))
            end = r + SUBLANES
            if end == hi or end % LANES == 0:
                new = _merge(slabs, lane_slab)
                if merged is not None:
                    new = jnp.where(lane_slab >= slabs[0][0], new, merged)
                merged, slabs = new, []
            if end % LANES == 0:
                mine.append(to_lanes(merged))
                send_buf[:, end - LANES:end] = mine[-1]
                merged = None
        if hi < tail:
            fence()
            n_fences += 1
        elif lo < tail:
            head_msg.start()
    tail_msg.start()

    raw_load = load(0, n_raw, len(chunks))
    raw_load.start()
    raw_load.wait()
    own = {r: fold(x_buf, r) for r in range(0, n_raw, SUBLANES)}
    both = None
    for msg, (lo, hi) in zip(raw_msgs, raw_pieces):
        msg.wait_recv()
        new = to_lanes(_merge(
            [slab(r, own[r] + fold(raw_buf, r)) for r in range(lo, hi, SUBLANES)],
            lane_slab))
        both = new if both is None else jnp.where(lane[:1] >= lo, new, both)
        out_ref[:, :LANES] = both
        fence()
        n_fences += 1

    head_msg.wait_recv()
    for c in range(0, tail, LANES):
        total = mine[c // LANES] + recv_buf[:, c:c + LANES]
        if c == 0:
            total = jnp.where(lane[:1] < n_raw, both, total)
        out_ref[:, c:c + LANES] = total

    for msg in (*raw_msgs, head_msg, tail_msg):
        msg.wait_send()
    pl.semaphore_wait(fence_sem, n_fences)
    tail_msg.wait_recv()
    out_ref[:, tail:] = mine[-1] + recv_buf[:, tail:]


def pallas_dist_sum_ax1_xy_m512_n256_kernel(x: jax.Array):
    m, n = x.shape
    assert m == CHUNK_ENDS[-1] and n % LANES == 0, x.shape
    n_msgs = 2 + len(RAW_ENDS)
    out = pl.pallas_call(
        _kernel,
        out_shape=jax.ShapeDtypeStruct((1, m), x.dtype),
        in_specs=[pl.BlockSpec(memory_space=pltpu.HBM)],
        out_specs=pl.BlockSpec(memory_space=pltpu.VMEM),
        scratch_shapes=[
            pltpu.VMEM((m, n), x.dtype),
            pltpu.VMEM((RAW_ENDS[-1], n), x.dtype),
            pltpu.VMEM((1, m), x.dtype),
            pltpu.VMEM((1, m), x.dtype),
            pltpu.SemaphoreType.DMA((len(CHUNK_ENDS) + 1,)),
            pltpu.SemaphoreType.DMA((n_msgs,)),
            pltpu.SemaphoreType.DMA((n_msgs,)),
            pltpu.SemaphoreType.REGULAR,
        ],
        compiler_params=pltpu.CompilerParams(
            collective_id=0,
            disable_semaphore_checks=True,
            flags={"XLA_TPU_RESCHEDULE_DMA_DONES": True} if OVERLAP_WAITS else None,
        ),
    )(x)
    return out.reshape(m, 1)
```

```python
import functools

import jax
import jax.numpy as jnp
from jax import lax
from jax.experimental import pallas as pl
from jax.experimental.pallas import tpu as pltpu

SUBLANES, LANES = 8, 128

OVERLAP_WAITS = jax.__version_info__ >= (0, 12)

RAW_ENDS = (24, 32)
EARLY_ENDS = (176, 272)
LATE_ENDS = (360, 384, 432, 456, 480, 496, 504, 512) if OVERLAP_WAITS else (352, 440, 512)
CHUNK_ENDS = EARLY_ENDS + LATE_ENDS


def _merge(slabs, lane_slab):
    if len(slabs) == 1:
        return slabs[0][1]
    half = len(slabs) // 2
    return jnp.where(
        lane_slab >= slabs[half][0],
        _merge(slabs[half:], lane_slab),
        _merge(slabs[:half], lane_slab),
    )


def _kernel(x_hbm, out_ref, x_buf, raw_buf, send_buf, recv_buf,
            load_sems, send_sems, recv_sems, fence_sem):
    m, n = x_hbm.shape
    n_raw = RAW_ENDS[-1]
    chunks = list(zip((n_raw, *CHUNK_ENDS), CHUNK_ENDS))
    raw_pieces = list(zip((0, *RAW_ENDS), RAW_ENDS))

    def load(lo, hi, i):
        rows = pl.ds(lo, hi - lo)
        return pltpu.make_async_copy(x_hbm.at[rows], x_buf.at[rows], load_sems.at[i])

    loads = [load(lo, hi, i) for i, (lo, hi) in enumerate(chunks)]
    for copy in loads:
        copy.start()

    peer = (lax.axis_index("x"), 1 - lax.axis_index("y"))

    def to_peer(src, dst, i):
        return pltpu.make_async_remote_copy(
            src, dst, send_sems.at[i], recv_sems.at[i],
            device_id=peer, device_id_type=pl.DeviceIdType.MESH)

    raw_msgs = [
        to_peer(x_hbm.at[pl.ds(lo, hi - lo)], raw_buf.at[pl.ds(lo, hi - lo)], i)
        for i, (lo, hi) in enumerate(raw_pieces)
    ]
    sum_msgs = [
        to_peer(send_buf.at[i], recv_buf.at[i], len(raw_msgs) + i)
        for i in range(m // LANES)
    ]

    barrier = pltpu.get_barrier_semaphore()
    pl.semaphore_signal(barrier, device_id=peer, device_id_type=pl.DeviceIdType.MESH)
    pl.semaphore_wait(barrier)
    raw_msgs[0].start()

    lane = lax.broadcasted_iota(jnp.int32, (SUBLANES, LANES), 1)
    lane_slab, lane_row = lane >> 3, lane & 7

    def fold(ref, r):
        tiles = [ref[r:r + SUBLANES, c:c + LANES] for c in range(0, n, LANES)]
        return functools.reduce(jnp.add, tiles)

    def slab(r, folded):
        sums = jnp.sum(folded, axis=1, keepdims=True)
        return r % LANES // SUBLANES, jnp.broadcast_to(sums, (SUBLANES, LANES))

    def to_lanes(merged):
        return jnp.take_along_axis(merged, lane_row, axis=0)[:1]

    def fence():
        pl.semaphore_signal(fence_sem)

    mine, merged = [], None
    for copy, (lo, hi) in zip(loads, chunks):
        copy.wait()
        if hi == EARLY_ENDS[-1]:
            raw_msgs[1].start()
        slabs = []
        for r in range(lo, hi, SUBLANES):
            folded = fold(x_buf, r)
            if hi in LATE_ENDS and hi % LANES:
                x_buf[r:r + SUBLANES, :LANES] = folded
            slabs.append(slab(r, folded))
            end = r + SUBLANES
            if end == hi or end % LANES == 0:
                new = _merge(slabs, lane_slab)
                if merged is not None:
                    new = jnp.where(lane_slab >= slabs[0][0], new, merged)
                merged, slabs = new, []
            if end % LANES == 0:
                mine.append(to_lanes(merged))
                send_buf[r // LANES] = mine[-1]
                merged = None
        for msg in sum_msgs[lo // LANES:hi // LANES]:
            msg.start()
        if hi in EARLY_ENDS:
            fence()

    raw_load = load(0, n_raw, len(chunks))
    raw_load.start()
    raw_load.wait()
    own = {r: fold(x_buf, r) for r in range(0, n_raw, SUBLANES)}
    both = None
    for msg, (lo, hi) in zip(raw_msgs, raw_pieces):
        msg.wait_recv()
        new = to_lanes(_merge(
            [slab(r, own[r] + fold(raw_buf, r)) for r in range(lo, hi, SUBLANES)],
            lane_slab))
        both = new if both is None else jnp.where(lane[:1] >= lo, new, both)
        out_ref[:, :LANES] = both
        fence()

    for i, msg in enumerate(sum_msgs):
        if msg is sum_msgs[-1]:
            for sent in raw_msgs + sum_msgs:
                sent.wait_send()
            pl.semaphore_wait(fence_sem, len(EARLY_ENDS) + len(raw_msgs))
        msg.wait_recv()
        total = mine[i] + recv_buf[i]
        if i == 0:
            total = jnp.where(lane[:1] < n_raw, both, total)
        out_ref[:, i * LANES:(i + 1) * LANES] = total


def pallas_dist_sum_ax1_xy_m512_n256_kernel(x: jax.Array):
    m, n = x.shape
    assert m == CHUNK_ENDS[-1] and n % LANES == 0, x.shape
    n_msgs = len(RAW_ENDS) + m // LANES
    out = pl.pallas_call(
        _kernel,
        out_shape=jax.ShapeDtypeStruct((1, m), x.dtype),
        in_specs=[pl.BlockSpec(memory_space=pltpu.HBM)],
        out_specs=pl.BlockSpec(memory_space=pltpu.VMEM),
        scratch_shapes=[
            pltpu.VMEM((m, n), x.dtype),
            pltpu.VMEM((RAW_ENDS[-1], n), x.dtype),
            pltpu.VMEM((m // LANES, 1, LANES), x.dtype),
            pltpu.VMEM((m // LANES, 1, LANES), x.dtype),
            pltpu.SemaphoreType.DMA((len(CHUNK_ENDS) + 1,)),
            pltpu.SemaphoreType.DMA((n_msgs,)),
            pltpu.SemaphoreType.DMA((n_msgs,)),
            pltpu.SemaphoreType.REGULAR,
        ],
        compiler_params=pltpu.CompilerParams(
            collective_id=0,
            disable_semaphore_checks=True,
            flags={"XLA_TPU_RESCHEDULE_DMA_DONES": True} if OVERLAP_WAITS else None,
        ),
    )(x)
    return out.reshape(m, 1)
```
